```python
import numpy as np

kernel_name = "dist_layernorm_xy_m6144_n2048"

def setup_inputs():
    x = np.random.randn(12288, 4096).astype(np.float32)
    gamma = np.random.randn(4096).astype(np.float32)
    beta = np.random.randn(4096).astype(np.float32)
    return {"x": x, "gamma": gamma, "beta": beta}

def reference(x: np.ndarray, gamma: np.ndarray, beta: np.ndarray) -> np.ndarray:
    eps = 1e-5
    mean = np.mean(x, axis=1, keepdims=True)
    var = np.var(x, axis=1, keepdims=True)
    return gamma * (x - mean) / np.sqrt(var + eps) + beta
```

```python
import contextlib
import os
import jax
import jax.numpy as jnp
from jax import lax
from jax.experimental import pallas as pl
from jax.experimental.pallas import tpu as pltpu

M, N = 6144, 2048
N_GLOBAL = 2 * N
EPS = 1e-5
K = N // 128
RUNS = tuple(tuple(int(a) for a in v.split("x")) for v in os.environ.get("K_RUNS", "512x10,256x3").split(","))
TAIL = tuple(int(v) for v in os.environ.get("K_TAIL", "128,64,32,32").split(",") if v)
SIZES = [r for r, n in RUNS for _ in range(n)] + list(TAIL)
assert sum(SIZES) == M
NC = len(SIZES)
STARTS = [sum(SIZES[:i]) for i in range(NC)]
DEPTH = int(os.environ.get("K_D", 4))
EARLY_FIN = int(os.environ.get("K_EF", 0))
SCOPES = os.environ.get("K_SCOPES", "0") == "1"
ODT = {"f32": jnp.float32, "bf16": jnp.bfloat16}[os.environ.get("K_ODT", "bf16")]


def scope(n):
    return jax.named_scope(n) if SCOPES else contextlib.nullcontext()


def pallas_dist_layernorm_xy_m6144_n2048_kernel(x, gamma, beta):
    def body(x_hbm, g_hbm, b_hbm, o_ref, xbuf, g_ref, b_ref, g8, b8, sbuf, rbuf,
             ld_sems, gb_sem, send_sem, recv_sems):
        my_x = lax.axis_index("x")
        my_y = lax.axis_index("y")
        nbr = (my_x, 1 - my_y)

        def load(c, start, rows):
            sl = pl.ds(start, rows)
            return pltpu.make_async_copy(x_hbm.at[sl], xbuf.at[sl], ld_sems.at[c % DEPTH])

        def exchange(c):
            return pltpu.make_async_remote_copy(
                src_ref=sbuf.at[c], dst_ref=rbuf.at[c],
                send_sem=send_sem, recv_sem=recv_sems.at[c],
                device_id=nbr, device_id_type=pl.DeviceIdType.MESH)

        g_copy = pltpu.make_async_copy(g_hbm, g_ref, gb_sem)
        b_copy = pltpu.make_async_copy(b_hbm, b_ref, gb_sem)
        g_copy.start()
        b_copy.start()
        for c in range(DEPTH):
            load(c, STARTS[c], SIZES[c]).start()

        barrier = pltpu.get_barrier_semaphore()
        pl.semaphore_signal(barrier, inc=1, device_id=nbr,
                            device_id_type=pl.DeviceIdType.MESH)
        g_copy.wait()
        b_copy.wait()
        g8[...] = jnp.broadcast_to(g_ref[...], g8.shape)
        b8[...] = jnp.broadcast_to(b_ref[...], b8.shape)
        pl.semaphore_wait(barrier, 1)

        lane = lax.broadcasted_iota(jnp.int32, (16, 128), 1)

        def stats(c, start, rows):
            packed = jnp.zeros((16, 128), jnp.float32)
            for j in range(rows // 16):
                xs = xbuf[pl.ds(start + j * 16, 16), :]
                m = jnp.sum(xs, axis=1, keepdims=True) * (1.0 / N)
                d = xs - m
                v = jnp.sum(d * d, axis=1, keepdims=True)
                packed = jnp.where(lane == j, m, jnp.where(lane == 64 + j, v, packed))
            sbuf[c] = packed

        def normalize(c, start, rows):
            mine, theirs = sbuf[c], rbuf[c]
            mean = (mine + theirs) * 0.5
            dm = mine - theirs
            m2 = pltpu.roll(mine + theirs, 64, axis=1)
            var = (m2 + dm * dm * (0.5 * N)) * (1.0 / N_GLOBAL)
            rstd = lax.rsqrt(var + EPS)
            g2 = jnp.concatenate([g8[...], g8[...]], axis=0)
            b2 = jnp.concatenate([b8[...], b8[...]], axis=0)
            for j in range(rows // 16):
                hit = lane == j
                mg = jnp.sum(jnp.where(hit, mean, 0.0), axis=1, keepdims=True)
                rg = jnp.sum(jnp.where(hit, rstd, 0.0), axis=1, keepdims=True)
                sl = pl.ds(start + j * 16, 16)
                y = (xbuf[sl, :] - mg) * rg * g2 + b2
                o_ref[sl, :] = y.astype(ODT)

        def arrive(c, start, rows, nxt):
            with scope("ldwait"):
                load(c, start, rows).wait()
            nxt()
            with scope("stats"):
                stats(c, start, rows)
                exchange(c).start()

        def finish(c, start, rows):
            with scope("recv"):
                exchange(c).wait_recv()
            with scope("norm"):
                normalize(c, start, rows)

        def refill_static(c):
            def go():
                if c + DEPTH < NC:
                    load(c + DEPTH, STARTS[c + DEPTH], SIZES[c + DEPTH]).start()
            return go

        c0 = 0
        prev_rows = None
        for rows, count in RUNS:
            start0 = STARTS[c0]
            arrive(c0, start0, rows, refill_static(c0))
            if prev_rows is not None:
                finish(c0 - 1, STARTS[c0 - 1], prev_rows)

            def step(i, _, c0=c0, rows=rows, count=count, start0=start0):
                c = c0 + i
                start = pl.multiple_of(start0 + i * rows, 16)

                def refill():
                    @pl.when(i + DEPTH < count)
                    def _():
                        load(c + DEPTH, pl.multiple_of(start0 + (i + DEPTH) * rows, 16), rows).start()
                    for k in range(max(1, count - DEPTH), count):
                        t = c0 + k + DEPTH
                        if t < NC:
                            @pl.when(i == k)
                            def _(t=t):
                                load(t, STARTS[t], SIZES[t]).start()
                arrive(c, start, rows, refill)
                finish(c - 1, pl.multiple_of(start0 + (i - 1) * rows, 16), rows)
                return 0
            lax.fori_loop(1, count, step, 0)
            c0 += count
            prev_rows = rows

        pend = [c0 - 1]
        for i in range(len(TAIL)):
            c = c0 + i
            arrive(c, STARTS[c], SIZES[c], refill_static(c))
            if i < EARLY_FIN:
                p = pend.pop(0)
                finish(p, STARTS[p], SIZES[p])
            pend.append(c)
        for p in pend:
            finish(p, STARTS[p], SIZES[p])

        pltpu.make_async_remote_copy(
            src_ref=sbuf, dst_ref=rbuf, send_sem=send_sem, recv_sem=recv_sems.at[0],
            device_id=nbr, device_id_type=pl.DeviceIdType.MESH).wait_send()

    return pl.pallas_call(
        body,
        out_shape=pltpu.VMEM((M, N), ODT),
        in_specs=[pl.BlockSpec(memory_space=pl.ANY),
                  pl.BlockSpec(memory_space=pl.ANY),
                  pl.BlockSpec(memory_space=pl.ANY)],
        out_specs=pl.BlockSpec(memory_space=pltpu.VMEM),
        scratch_shapes=[
            pltpu.VMEM((M, N), jnp.float32),
            pltpu.VMEM((1, N), jnp.float32),
            pltpu.VMEM((1, N), jnp.float32),
            pltpu.VMEM((8, N), jnp.float32),
            pltpu.VMEM((8, N), jnp.float32),
            pltpu.VMEM((NC, 16, 128), jnp.float32),
            pltpu.VMEM((NC, 16, 128), jnp.float32),
            pltpu.SemaphoreType.DMA((DEPTH,)),
            pltpu.SemaphoreType.DMA,
            pltpu.SemaphoreType.DMA,
            pltpu.SemaphoreType.DMA((NC,)),
        ],
        compiler_params=pltpu.CompilerParams(
            collective_id=0, vmem_limit_bytes=52 * 1024 * 1024),
    )(x, gamma.reshape(1, N), beta.reshape(1, N))
```

```python
import jax
import jax.numpy as jnp
from jax import lax
from jax.experimental import pallas as pl
from jax.experimental.pallas import tpu as pltpu

M, N = 6144, 2048
N_GLOBAL = 2 * N
EPS = 1e-5
OUT_DTYPE = jnp.bfloat16

GROUP = 16
RUNS = ((512, 10), (256, 3))
TAIL = (128, 64, 32, 32)
SIZES = tuple(r for r, n in RUNS for _ in range(n)) + TAIL
STARTS = tuple(sum(SIZES[:i]) for i in range(len(SIZES)))
NC = len(SIZES)
DEPTH = 4
assert sum(SIZES) == M and all(r % GROUP == 0 and r // GROUP <= 64 for r in SIZES)


def pallas_dist_layernorm_xy_m6144_n2048_kernel(
    x: jax.Array,
    gamma: jax.Array,
    beta: jax.Array,
):
    def body(x_hbm, g_hbm, b_hbm, o_ref, xbuf, g_row, b_row, g8, b8, sbuf, rbuf,
             ld_sems, gb_sem, send_sem, recv_sems):
        nbr = (lax.axis_index("x"), 1 - lax.axis_index("y"))

        def load(c, start, rows):
            sl = pl.ds(start, rows)
            return pltpu.make_async_copy(x_hbm.at[sl], xbuf.at[sl], ld_sems.at[c % DEPTH])

        def exchange(c):
            return pltpu.make_async_remote_copy(
                src_ref=sbuf.at[c], dst_ref=rbuf.at[c],
                send_sem=send_sem, recv_sem=recv_sems.at[c],
                device_id=nbr, device_id_type=pl.DeviceIdType.MESH)

        g_copy = pltpu.make_async_copy(g_hbm, g_row, gb_sem)
        b_copy = pltpu.make_async_copy(b_hbm, b_row, gb_sem)
        g_copy.start()
        b_copy.start()
        for c in range(DEPTH):
            load(c, STARTS[c], SIZES[c]).start()

        barrier = pltpu.get_barrier_semaphore()
        pl.semaphore_signal(barrier, inc=1, device_id=nbr,
                            device_id_type=pl.DeviceIdType.MESH)
        g_copy.wait()
        b_copy.wait()
        g8[...] = jnp.broadcast_to(g_row[...], g8.shape)
        b8[...] = jnp.broadcast_to(b_row[...], b8.shape)
        pl.semaphore_wait(barrier, 1)

        lane = lax.broadcasted_iota(jnp.int32, (GROUP, 128), 1)

        def stats(c, start, rows):
            packed = jnp.zeros((GROUP, 128), jnp.float32)
            for j in range(rows // GROUP):
                xs = xbuf[pl.ds(start + j * GROUP, GROUP), :]
                m = jnp.sum(xs, axis=1, keepdims=True) * (1.0 / N)
                d = xs - m
                m2 = jnp.sum(d * d, axis=1, keepdims=True)
                packed = jnp.where(lane == j, m, jnp.where(lane == 64 + j, m2, packed))
            sbuf[c] = packed

        def normalize(c, start, rows):
            mine, theirs = sbuf[c], rbuf[c]
            mean = (mine + theirs) * 0.5
            dm = mine - theirs
            m2 = pltpu.roll(mine + theirs, 64, axis=1)
            var = (m2 + dm * dm * (0.5 * N)) * (1.0 / N_GLOBAL)
            rstd = lax.rsqrt(var + EPS)
            g2 = jnp.concatenate([g8[...], g8[...]], axis=0)
            b2 = jnp.concatenate([b8[...], b8[...]], axis=0)
            for j in range(rows // GROUP):
                hit = lane == j
                mg = jnp.sum(jnp.where(hit, mean, 0.0), axis=1, keepdims=True)
                rg = jnp.sum(jnp.where(hit, rstd, 0.0), axis=1, keepdims=True)
                sl = pl.ds(start + j * GROUP, GROUP)
                y = (xbuf[sl, :] - mg) * rg * g2 + b2
                o_ref[sl, :] = y.astype(OUT_DTYPE)

        def arrive(c, start, rows, refill):
            load(c, start, rows).wait()
            refill()
            stats(c, start, rows)
            exchange(c).start()

        def finish(c, start, rows):
            exchange(c).wait_recv()
            normalize(c, start, rows)

        def refill_static(c):
            def go():
                if c + DEPTH < NC:
                    load(c + DEPTH, STARTS[c + DEPTH], SIZES[c + DEPTH]).start()
            return go

        c0 = 0
        for rows, count in RUNS:
            start0 = STARTS[c0]
            arrive(c0, start0, rows, refill_static(c0))
            if c0 > 0:
                finish(c0 - 1, STARTS[c0 - 1], SIZES[c0 - 1])

            def step(i, _, c0=c0, rows=rows, count=count, start0=start0):
                def at(k):
                    return pl.multiple_of(start0 + k * rows, GROUP)

                def refill():
                    @pl.when(i + DEPTH < count)
                    def _():
                        load(c0 + i + DEPTH, at(i + DEPTH), rows).start()

                    for k in range(max(1, count - DEPTH), count):
                        t = c0 + k + DEPTH
                        if t < NC:
                            @pl.when(i == k)
                            def _(t=t):
                                load(t, STARTS[t], SIZES[t]).start()

                arrive(c0 + i, at(i), rows, refill)
                finish(c0 + i - 1, at(i - 1), rows)
                return 0

            lax.fori_loop(1, count, step, 0)
            c0 += count

        for c in range(c0, NC):
            arrive(c, STARTS[c], SIZES[c], refill_static(c))
        for c in range(c0 - 1, NC):
            finish(c, STARTS[c], SIZES[c])

        pltpu.make_async_remote_copy(
            src_ref=sbuf, dst_ref=rbuf, send_sem=send_sem, recv_sem=recv_sems.at[0],
            device_id=nbr, device_id_type=pl.DeviceIdType.MESH).wait_send()

    return pl.pallas_call(
        body,
        out_shape=pltpu.VMEM((M, N), OUT_DTYPE),
        in_specs=[pl.BlockSpec(memory_space=pl.ANY)] * 3,
        out_specs=pl.BlockSpec(memory_space=pltpu.VMEM),
        scratch_shapes=[
            pltpu.VMEM((M, N), jnp.float32),
            pltpu.VMEM((1, N), jnp.float32),
            pltpu.VMEM((1, N), jnp.float32),
            pltpu.VMEM((8, N), jnp.float32),
            pltpu.VMEM((8, N), jnp.float32),
            pltpu.VMEM((NC, GROUP, 128), jnp.float32),
            pltpu.VMEM((NC, GROUP, 128), jnp.float32),
            pltpu.SemaphoreType.DMA((DEPTH,)),
            pltpu.SemaphoreType.DMA,
            pltpu.SemaphoreType.DMA,
            pltpu.SemaphoreType.DMA((NC,)),
        ],
        compiler_params=pltpu.CompilerParams(
            collective_id=0, vmem_limit_bytes=52 * 1024 * 1024),
    )(x, gamma.reshape(1, N), beta.reshape(1, N))
```

```python
import jax
import jax.numpy as jnp
from jax import lax
from jax.experimental import pallas as pl
from jax.experimental.pallas import tpu as pltpu

M, N = 6144, 2048
N_GLOBAL = 2 * N
EPS = 1e-5
OUT_DTYPE = jnp.float32

GROUP = 16
RUNS = ((512, 10), (256, 3))
TAIL = (128, 64, 32, 32)
SIZES = tuple(r for r, n in RUNS for _ in range(n)) + TAIL
STARTS = tuple(sum(SIZES[:i]) for i in range(len(SIZES)))
NC = len(SIZES)
DEPTH = 4
assert RUNS[0][1] >= DEPTH
assert sum(SIZES) == M and all(r % GROUP == 0 and r // GROUP <= 64 for r in SIZES)


def pallas_dist_layernorm_xy_m6144_n2048_kernel(
    x: jax.Array,
    gamma: jax.Array,
    beta: jax.Array,
):
    def body(x_hbm, g_hbm, b_hbm, o_ref, xbuf, g_row, b_row, g8, b8, sbuf, rbuf,
             ld_sems, gb_sem, send_sem, recv_sems):
        nbr = (lax.axis_index("x"), 1 - lax.axis_index("y"))

        def load(c, start, rows):
            sl = pl.ds(start, rows)
            return pltpu.make_async_copy(x_hbm.at[sl], xbuf.at[sl], ld_sems.at[c % DEPTH])

        def exchange(c):
            return pltpu.make_async_remote_copy(
                src_ref=sbuf.at[c], dst_ref=rbuf.at[c],
                send_sem=send_sem, recv_sem=recv_sems.at[c],
                device_id=nbr, device_id_type=pl.DeviceIdType.MESH)

        g_copy = pltpu.make_async_copy(g_hbm, g_row, gb_sem)
        b_copy = pltpu.make_async_copy(b_hbm, b_row, gb_sem)
        g_copy.start()
        b_copy.start()

        def first_loads(c, _):
            load(c, pl.multiple_of(c * RUNS[0][0], GROUP), RUNS[0][0]).start()
            return 0

        lax.fori_loop(0, DEPTH, first_loads, 0)

        barrier = pltpu.get_barrier_semaphore()
        pl.semaphore_signal(barrier, inc=1, device_id=nbr,
                            device_id_type=pl.DeviceIdType.MESH)
        g_copy.wait()
        b_copy.wait()
        g8[...] = jnp.broadcast_to(g_row[...], g8.shape)
        b8[...] = jnp.broadcast_to(b_row[...], b8.shape)
        pl.semaphore_wait(barrier, 1)

        lane = lax.broadcasted_iota(jnp.int32, (GROUP, 128), 1)

        def stats(c, start, rows):
            packed = jnp.zeros((GROUP, 128), jnp.float32)
            for j in range(rows // GROUP):
                xs = xbuf[pl.ds(start + j * GROUP, GROUP), :]
                m = jnp.sum(xs, axis=1, keepdims=True) * (1.0 / N)
                d = xs - m
                m2 = jnp.sum(d * d, axis=1, keepdims=True)
                packed = jnp.where(lane == j, m, jnp.where(lane == 64 + j, m2, packed))
            sbuf[c] = packed

        def normalize(c, start, rows):
            mine, theirs = sbuf[c], rbuf[c]
            mean = (mine + theirs) * 0.5
            dm = mine - theirs
            m2 = pltpu.roll(mine + theirs, 64, axis=1)
            var = (m2 + dm * dm * (0.5 * N)) * (1.0 / N_GLOBAL)
            rstd = lax.rsqrt(var + EPS)
            g2 = jnp.concatenate([g8[...], g8[...]], axis=0)
            b2 = jnp.concatenate([b8[...], b8[...]], axis=0)
            for j in range(rows // GROUP):
                hit = lane == j
                mg = jnp.sum(jnp.where(hit, mean, 0.0), axis=1, keepdims=True)
                rg = jnp.sum(jnp.where(hit, rstd, 0.0), axis=1, keepdims=True)
                sl = pl.ds(start + j * GROUP, GROUP)
                y = (xbuf[sl, :] - mg) * rg * g2 + b2
                o_ref[sl, :] = y.astype(OUT_DTYPE)

        def arrive(c, start, rows, refill):
            load(c, start, rows).wait()
            refill()
            stats(c, start, rows)
            exchange(c).start()

        def finish(c, start, rows):
            exchange(c).wait_recv()
            normalize(c, start, rows)

        def refill_static(c):
            def go():
                if c + DEPTH < NC:
                    load(c + DEPTH, STARTS[c + DEPTH], SIZES[c + DEPTH]).start()
            return go

        c0 = 0
        for rows, count in RUNS:
            start0 = STARTS[c0]
            arrive(c0, start0, rows, refill_static(c0))
            if c0 > 0:
                finish(c0 - 1, STARTS[c0 - 1], SIZES[c0 - 1])

            def step(i, _, c0=c0, rows=rows, count=count, start0=start0):
                def at(k):
                    return pl.multiple_of(start0 + k * rows, GROUP)

                def refill():
                    @pl.when(i + DEPTH < count)
                    def _():
                        load(c0 + i + DEPTH, at(i + DEPTH), rows).start()

                    for k in range(max(1, count - DEPTH), count):
                        t = c0 + k + DEPTH
                        if t < NC:
                            @pl.when(i == k)
                            def _(t=t):
                                load(t, STARTS[t], SIZES[t]).start()

                arrive(c0 + i, at(i), rows, refill)
                finish(c0 + i - 1, at(i - 1), rows)
                return 0

            lax.fori_loop(1, count, step, 0)
            c0 += count

        for c in range(c0, NC):
            arrive(c, STARTS[c], SIZES[c], refill_static(c))
        for c in range(c0 - 1, NC):
            finish(c, STARTS[c], SIZES[c])

        pltpu.make_async_remote_copy(
            src_ref=sbuf, dst_ref=rbuf, send_sem=send_sem, recv_sem=recv_sems.at[0],
            device_id=nbr, device_id_type=pl.DeviceIdType.MESH).wait_send()

    return pl.pallas_call(
        body,
        out_shape=pltpu.VMEM((M, N), OUT_DTYPE),
        in_specs=[pl.BlockSpec(memory_space=pl.ANY)] * 3,
        out_specs=pl.BlockSpec(memory_space=pltpu.VMEM),
        scratch_shapes=[
            pltpu.VMEM((M, N), jnp.float32),
            pltpu.VMEM((1, N), jnp.float32),
            pltpu.VMEM((1, N), jnp.float32),
            pltpu.VMEM((8, N), jnp.float32),
            pltpu.VMEM((8, N), jnp.float32),
            pltpu.VMEM((NC, GROUP, 128), jnp.float32),
            pltpu.VMEM((NC, GROUP, 128), jnp.float32),
            pltpu.SemaphoreType.DMA((DEPTH,)),
            pltpu.SemaphoreType.DMA,
            pltpu.SemaphoreType.DMA,
            pltpu.SemaphoreType.DMA((NC,)),
        ],
        compiler_params=pltpu.CompilerParams(
            collective_id=0, vmem_limit_bytes=52 * 1024 * 1024),
    )(x, gamma.reshape(1, N), beta.reshape(1, N))
```
